```python
import numpy as np

kernel_name = "dist_f_of_ar_i_m4096_n1024"

def setup_inputs():
    t = np.random.randn(16384, 1024).astype(np.float32)
    return {"t": t}

def reference(t: np.ndarray) -> np.ndarray:
    s = t.reshape(4, 4096, 1024).sum(axis=0)
    r = np.maximum(s, 0.0)
    return np.tanh(s) * s * s + r * r * r
```

```python
import functools
import jax
import jax.numpy as jnp
from jax import lax
from jax.experimental import pallas as pl
from jax.experimental.pallas import tpu as pltpu

F32, BF16 = jnp.float32, jnp.bfloat16


def _bounds(sizes, total):
    out, r = [], 0
    for s in sizes:
        out.append((r, s)); r += s
    assert r == total, (sizes, total)
    return out


def make(p1=(32, 96, 320, 576), after1=(3, 4), p3=(448, 400, 128, 32, 16), step=32, nobc=False):
    def fn(t):
        m, n = t.shape
        q = m // 4
        c1 = _bounds(p1, q)
        c2, first = [], 0
        for last in after1:
            c2.append((c1[first][0], sum(s for _, s in c1[first:last]), range(first, last))); first = last
        c3 = _bounds(p3, q)
        n1, n2, n3 = len(c1), len(c2), len(c3)
        nd = n1 + n2 + n3

        def body(t_ref, o_ref, stage, sbuf, rbuf, in_sems, out_sems, ssems, rsems):
            me = lax.axis_index("i")
            peer = (me ^ 1, 3 - me)
            side = (((me + 1) >> 1) & 1, me >> 1)
            keep = [(2 * h + side[h]) * q for h in range(2)]
            give = [(2 * h + 1 - side[h]) * q for h in range(2)]

            bar = pltpu.get_barrier_semaphore()
            for p in peer:
                pl.semaphore_signal(bar, inc=1, device_id=(p,), device_id_type=pl.DeviceIdType.MESH)

            def load(slot, base, r0, rows, k):
                return pltpu.make_async_copy(
                    t_ref.at[pl.ds(pl.multiple_of(base + r0, 16), rows)], stage.at[slot, pl.ds(r0, rows)], in_sems.at[k])

            def store(slot, base, r0, rows, k):
                return pltpu.make_async_copy(
                    stage.at[slot, pl.ds(r0, rows)], o_ref.at[pl.ds(pl.multiple_of(base + r0, 16), rows)], out_sems.at[k])

            def hop(l, k, r0, rows):
                return pltpu.make_async_remote_copy(
                    sbuf.at[l, pl.ds(r0, rows)], rbuf.at[l, pl.ds(r0, rows)],
                    ssems.at[l * nd + k], rsems.at[l * nd + k],
                    device_id=(peer[l],), device_id_type=pl.DeviceIdType.MESH)

            def rows_loop(r0, rows, f):
                st = min(step, rows)
                while rows % st: st -= 16
                if rows == st:
                    f(r0, st)
                else:
                    @pl.loop(0, rows // st)
                    def _(i):
                        f(pl.multiple_of(r0 + i * st, 16), st)

            gl = [[load(l, give[l], r0, rows, l * n1 + k) for l in range(2)] for k, (r0, rows) in enumerate(c1)]
            kl = [[load(2 + h, keep[h], r0, rows, 2 * n1 + h * n2 + k) for h in range(2)] for k, (r0, rows, _) in enumerate(c2)]
            for pair in gl + kl:
                for c in pair: c.start()
            sends, stores = [], []

            for k, (r0, rows) in enumerate(c1):
                for l in range(2):
                    gl[k][l].wait()
                    def f(r, st, l=l):
                        sbuf[l, pl.ds(r, st), :] = stage[l, pl.ds(r, st), :].astype(BF16)
                    rows_loop(r0, rows, f)
                    if k > 0:
                        c = hop(l, k, r0, rows); c.start(); sends.append(c)
                if k == 0:
                    pl.semaphore_wait(bar, 2)
                    for l in range(2):
                        c = hop(l, k, r0, rows); c.start(); sends.append(c)

            for k, (r0, rows, deps) in enumerate(c2):
                for l in range(2):
                    h = 1 - l
                    kl[k][h].wait()
                    for d in deps:
                        hop(h, d, *c1[d]).wait_recv()
                    def f(r, st, l=l, h=h):
                        s = stage[2 + h, pl.ds(r, st), :] + rbuf[h, pl.ds(r, st), :].astype(F32)
                        sbuf[l, pl.ds(q + r, st), :] = s.astype(BF16)
                    rows_loop(r0, rows, f)
                    c = hop(l, n1 + k, q + r0, rows); c.start(); sends.append(c)

            started = 0
            for k, (r0, rows, _) in enumerate(c2):
                ready = [j for j in range(started, n3) if c3[j][0] + c3[j][1] <= r0 + rows]
                for l in range(2):
                    h = 1 - l
                    hop(h, n1 + k, q + r0, rows).wait_recv()
                    def f(r, st, l=l, h=h):
                        s = sbuf[h, pl.ds(q + r, st), :].astype(F32) + rbuf[h, pl.ds(q + r, st), :].astype(F32)
                        p = jnp.maximum(s, 0.0)
                        y = (jnp.tanh(s) * s * s + p * p * p).astype(BF16)
                        sbuf[l, pl.ds(2 * q + r, st), :] = y
                        stage[2 + l, pl.ds(r, st), :] = y.astype(F32)
                    rows_loop(r0, rows, f)
                    for j in ready:
                        c = hop(l, n1 + n2 + j, 2 * q + c3[j][0], c3[j][1]); c.start(); sends.append(c)
                    c = store(2 + l, keep[l], r0, rows, l * n2 + k); c.start(); stores.append(c)
                started += len(ready)
            assert started == n3

            for k, (r0, rows) in enumerate(c3):
                for l in range(2):
                    hop(l, n1 + n2 + k, 2 * q + r0, rows).wait_recv()
                    def f(r, st, l=l):
                        stage[l, pl.ds(r, st), :] = rbuf[l, pl.ds(2 * q + r, st), :].astype(F32)
                    rows_loop(r0, rows, f)
                    c = store(l, give[l], r0, rows, 2 * n2 + l * n3 + k); c.start(); stores.append(c)
                if k == 0:
                    early, sends = sends[:2 * (n1 + n2)], sends[2 * (n1 + n2):]
                    for c in early: c.wait_send()
            for c in sends: c.wait_send()
            for c in stores: c.wait()

        return pl.pallas_call(
            body,
            out_shape=pltpu.HBM((m, n), F32),
            in_specs=[pl.BlockSpec(memory_space=pltpu.HBM)],
            out_specs=pl.BlockSpec(memory_space=pltpu.HBM),
            scratch_shapes=[
                pltpu.VMEM((4, q, n), F32),
                pltpu.VMEM((2, 3 * q, n), BF16),
                pltpu.VMEM((2, 3 * q, n), BF16),
                pltpu.SemaphoreType.DMA((2 * (n1 + n2),)),
                pltpu.SemaphoreType.DMA((2 * (n2 + n3),)),
                pltpu.SemaphoreType.DMA((2 * nd,)),
                pltpu.SemaphoreType.DMA((2 * nd,)),
            ],
            compiler_params=pltpu.CompilerParams(collective_id=0, vmem_limit_bytes=64 << 20, disable_bounds_checks=nobc),
        )(t)
    return fn


def pallas_dist_f_of_ar_i_m4096_n1024_kernel(t):
    return make()(t)
```

```python
import jax
import jax.numpy as jnp
from jax import lax
from jax.experimental import pallas as pl
from jax.experimental.pallas import tpu as pltpu

F32, BF16 = jnp.float32, jnp.bfloat16

ROWS, COLS = 4096, 1024
QUARTER = ROWS // 4
STEP = 32
GROUP = 128

PHASE1 = ((0, 32), (32, 96), (128, 384), (512, 512))
PHASE2 = ((0, 512), (512, 512))
PHASE3 = ((0, 512), (512, 480), (992, 32))


def _inside(chunks, outer):
    first, rows = outer
    found = [(k, c) for k, c in enumerate(chunks) if first <= c[0] < first + rows]
    assert found[0][1][0] == first and sum(c[1] for _, c in found) == rows
    return found


def _kernel(t_ref, out0_ref, out1_ref, give_buf, keep_buf, send_buf, recv_buf,
            give_sems, keep_sem, send_sem, recv1_sems, recv2_sems, recv3_sems):
    me = lax.axis_index("i")
    peer = (me ^ 1, 3 - me)
    side = (((me + 1) >> 1) & 1, me >> 1)
    keep_row = [side[h] * QUARTER for h in range(2)]
    give_row = [(1 - side[h]) * QUARTER for h in range(2)]

    barrier = pltpu.get_barrier_semaphore()
    for p in peer:
        pl.semaphore_signal(
            barrier, inc=1, device_id=(p,), device_id_type=pl.DeviceIdType.MESH)

    def load(row_in_half, buf, chunk, sem):
        first, rows = chunk
        for h in range(2):
            row = pl.multiple_of(2 * QUARTER * h + row_in_half[h] + first, STEP)
            pltpu.make_async_copy(
                t_ref.at[pl.ds(row, rows)], buf.at[h, pl.ds(first, rows)], sem
            ).start()

    def send(phase, chunk, recv_sem):
        rows = pl.ds(phase * QUARTER + chunk[0], chunk[1])
        for link in range(2):
            pltpu.make_async_remote_copy(
                send_buf.at[link, rows], recv_buf.at[link, rows], send_sem, recv_sem,
                device_id=(peer[link],), device_id_type=pl.DeviceIdType.MESH,
            ).start()

    def wait_for_all(buf, sem):
        pltpu.make_async_copy(buf, buf, sem).wait()

    def wait_recv(phase, chunk, recv_sem):
        rows = pl.ds(phase * QUARTER + chunk[0], chunk[1])
        wait_for_all(recv_buf.at[:, rows], recv_sem)

    def for_rows(chunk, body):
        @pl.loop(0, chunk[1] // STEP)
        def _(i):
            r = pl.multiple_of(chunk[0] + i * STEP, STEP)
            for h in range(2):
                body(h, r)

    def store_result(h, row, y):
        rows = pl.ds(pl.multiple_of(row % GROUP, STEP), STEP)
        (out0_ref, out1_ref)[h][row // GROUP, rows, :] = y.astype(F32)

    def pack_given(h, r):
        send_buf[h, pl.ds(r, STEP), :] = give_buf[h, pl.ds(r, STEP), :].astype(BF16)

    def add_pair(h, r):
        pair = keep_buf[h, pl.ds(r, STEP), :] + recv_buf[h, pl.ds(r, STEP), :].astype(F32)
        pair = pair.astype(BF16)
        send_buf[1 - h, pl.ds(QUARTER + r, STEP), :] = pair
        keep_buf[h, pl.ds(r, STEP), :] = pair.astype(F32)

    def apply_f(h, r):
        other = recv_buf[1 - h, pl.ds(QUARTER + r, STEP), :].astype(F32)
        s = keep_buf[h, pl.ds(r, STEP), :] + other
        relu = jnp.maximum(s, 0.0)
        y = (jnp.tanh(s) * s * s + relu * relu * relu).astype(BF16)
        send_buf[h, pl.ds(2 * QUARTER + r, STEP), :] = y
        store_result(h, keep_row[h] + r, y)

    def unpack_result(h, r):
        store_result(h, give_row[h] + r, recv_buf[h, pl.ds(2 * QUARTER + r, STEP), :])

    for k, chunk in enumerate(PHASE1):
        load(give_row, give_buf, chunk, give_sems.at[k])
    load(keep_row, keep_buf, (0, QUARTER), keep_sem)

    for k, chunk in enumerate(PHASE1):
        wait_for_all(give_buf.at[:, pl.ds(*chunk)], give_sems.at[k])
        for_rows(chunk, pack_given)
        if k == 0:
            pl.semaphore_wait(barrier, 2)
        send(0, chunk, recv1_sems.at[k])

    wait_for_all(keep_buf, keep_sem)
    for k, chunk in enumerate(PHASE2):
        for j, part in _inside(PHASE1, chunk):
            wait_recv(0, part, recv1_sems.at[j])
        for_rows(chunk, add_pair)
        send(1, chunk, recv2_sems.at[k])

    for k, chunk in enumerate(PHASE2):
        wait_recv(1, chunk, recv2_sems.at[k])
        for_rows(chunk, apply_f)
        for j, part in _inside(PHASE3, chunk):
            send(2, part, recv3_sems.at[j])

    for k, chunk in enumerate(PHASE3):
        wait_recv(2, chunk, recv3_sems.at[k])
        for_rows(chunk, unpack_result)

    wait_for_all(send_buf, send_sem)


def pallas_dist_f_of_ar_i_m4096_n1024_kernel(t: jax.Array):
    assert t.shape == (ROWS, COLS) and t.dtype == F32
    half = jax.ShapeDtypeStruct((ROWS // 2 // GROUP, GROUP, COLS), F32)
    halves = pl.pallas_call(
        _kernel,
        out_shape=[half, half],
        in_specs=[pl.BlockSpec(memory_space=pltpu.HBM)],
        out_specs=[pl.BlockSpec(memory_space=pltpu.VMEM)] * 2,
        scratch_shapes=[
            pltpu.VMEM((2, QUARTER, COLS), F32),
            pltpu.VMEM((2, QUARTER, COLS), F32),
            pltpu.VMEM((2, 3 * QUARTER, COLS), BF16),
            pltpu.VMEM((2, 3 * QUARTER, COLS), BF16),
            pltpu.SemaphoreType.DMA((len(PHASE1),)),
            pltpu.SemaphoreType.DMA,
            pltpu.SemaphoreType.DMA,
            pltpu.SemaphoreType.DMA((len(PHASE1),)),
            pltpu.SemaphoreType.DMA((len(PHASE2),)),
            pltpu.SemaphoreType.DMA((len(PHASE3),)),
        ],
        compiler_params=pltpu.CompilerParams(
            collective_id=0, vmem_limit_bytes=64 * 1024 * 1024),
    )(t)
    return jnp.concatenate(halves, axis=0).reshape(ROWS, COLS)
```
